```python
import numpy as np

kernel_name = "dist_moe_shared_ep_outshard_n512_d256_e2_h512"

def setup_inputs():
    x = np.random.randn(512, 256).astype(np.float32)
    router_W = np.random.randn(256, 8).astype(np.float32) * 0.1
    scores64 = x.astype(np.float64) @ router_W.astype(np.float64)
    route_idx = np.argsort(-scores64, axis=-1)[:, :1].astype(np.int32)
    expert_W = np.random.randn(8, 256, 512).astype(np.float32) * 0.02
    shared_W = np.random.randn(256, 512).astype(np.float32) * 0.02
    return {"x": x, "router_W": router_W, "route_idx": route_idx, "expert_W": expert_W, "shared_W": shared_W}

def reference(x, router_W, route_idx, expert_W, shared_W):
    scores = x @ router_W
    s_max = scores.max(axis=-1, keepdims=True)
    probs = np.exp(scores - s_max)
    probs = probs / probs.sum(axis=-1, keepdims=True)
    shared = x @ shared_W
    out = np.zeros((512, 512), dtype=np.float32)
    for i in range(512):
        e = int(route_idx[i, 0])
        out[i] = shared[i] + probs[i, e] * (x[i] @ expert_W[e])
    return out
```

```python
import jax
import jax.numpy as jnp
from jax import lax
from jax.experimental import pallas as pl
from jax.experimental.pallas import tpu as pltpu

N_DEV = 4
BLK = 128
CAP = 64
N_PASS = BLK // CAP
ALIGN = 16
KCH = 128


def pallas_dist_moe_shared_ep_outshard_n512_d256_e2_h512_kernel(x, router_W, route_idx, expert_W, shared_W):
    n_tok, d_model = x.shape
    h = shared_W.shape[1]
    n_exp = router_W.shape[1]
    e_loc = expert_W.shape[0]
    assert n_tok == N_DEV * BLK and e_loc == 2
    k_tot = e_loc * d_model
    n_kch = k_tot // KCH
    f32, bf16, i32 = jnp.float32, jnp.bfloat16, jnp.int32

    def iota(shape, dim):
        return lax.broadcasted_iota(i32, shape, dim)

    def body(x_hbm, rwt_hbm, r4_hbm, ew_hbm, sw_hbm, out_hbm,
             x_v, rwt_v, r4_v, w_v, sw_v, out_v, key_v, lhs_v, send_buf, recv_buf,
             in_sems, out_sem, send_sems, recv_sems):
        me = lax.axis_index("i")
        peer = [(me + k) % N_DEV for k in range(N_DEV)]

        barrier_sem = pltpu.get_barrier_semaphore()
        for k in range(1, N_DEV):
            pl.semaphore_signal(barrier_sem, inc=1, device_id=(peer[k],), device_id_type=pl.DeviceIdType.MESH)

        cp_r = pltpu.make_async_copy(r4_hbm, r4_v, in_sems.at[0])
        cp_x = pltpu.make_async_copy(x_hbm, x_v, in_sems.at[1])
        cp_w = [
            pltpu.make_async_copy(
                ew_hbm.at[c // (d_model // KCH), pl.ds((c % (d_model // KCH)) * KCH, KCH)],
                w_v.at[pl.ds(c * KCH, KCH)], in_sems.at[2 + c])
            for c in range(n_kch)
        ]
        cp_rw = pltpu.make_async_copy(rwt_hbm, rwt_v, in_sems.at[2 + n_kch])
        cp_s = pltpu.make_async_copy(sw_hbm, sw_v, in_sems.at[3 + n_kch])
        cp_r.start()
        cp_x.start()
        for c in cp_w:
            c.start()
        cp_rw.start()
        cp_s.start()

        cp_r.wait()
        r4 = r4_v[...]
        r_own = r4_v[pl.ds(me, 1), :]
        sub8 = iota((8, BLK), 0)
        rsel = jnp.broadcast_to(r_own, (8, BLK))
        for d in range(N_DEV):
            rsel = jnp.where(sub8 == d, jnp.broadcast_to(r4[d:d + 1, :], (8, BLK)), rsel)
        g8 = rsel >> 1
        e8 = rsel & 1
        tgt8 = jnp.where(sub8 < N_DEV, me, (me - (sub8 - N_DEV)) & (N_DEV - 1))
        m8 = g8 == tgt8
        m8f = m8.astype(f32)
        upper = (iota((BLK, BLK), 0) < iota((BLK, BLK), 1)).astype(bf16)
        cum8 = jnp.dot(m8f.astype(bf16), upper, preferred_element_type=f32).astype(i32)

        def row_count(row):
            return jnp.sum(jnp.where(sub8 == row, m8f, 0.0)).astype(i32)

        cnt_send = [row_count(peer[k]) for k in range(N_DEV)]
        cnt_recv = [row_count(N_DEV + k) for k in range(N_DEV)]

        def n_rows(cnt, p):
            c = jnp.clip(cnt - p * CAP, 0, CAP)
            return pl.multiple_of(((c + (ALIGN - 1)) // ALIGN) * ALIGN, ALIGN)

        for p in range(N_PASS):
            rel = cum8 - p * CAP
            ok = m8 & (rel >= 0) & (rel < CAP)
            key_v[p] = jnp.where(ok, rel + CAP * e8, -1)

        rank_own = jnp.sum(jnp.where(sub8 >= N_DEV, cum8 * m8.astype(i32), 0), axis=0, keepdims=True)
        slot_own = (me - (r_own >> 1)) & (N_DEV - 1)

        max_send = jnp.maximum(jnp.maximum(cnt_send[0], cnt_send[1]), jnp.maximum(cnt_send[2], cnt_send[3]))
        max_recv = jnp.maximum(jnp.maximum(cnt_recv[0], cnt_recv[1]), jnp.maximum(cnt_recv[2], cnt_recv[3]))

        def send_copy(p, k):
            n = n_rows(cnt_send[k], p)
            return pltpu.make_async_remote_copy(
                src_ref=send_buf.at[p, pl.ds((k - 1) * CAP, n)],
                dst_ref=recv_buf.at[p, pl.ds(k * CAP, n)],
                send_sem=send_sems.at[p, k - 1], recv_sem=recv_sems.at[p, k - 1],
                device_id=(peer[k],), device_id_type=pl.DeviceIdType.MESH)

        def recv_copy(p, k):
            n = n_rows(cnt_recv[k], p)
            return pltpu.make_async_remote_copy(
                src_ref=send_buf.at[p, pl.ds((k - 1) * CAP, n)],
                dst_ref=recv_buf.at[p, pl.ds(k * CAP, n)],
                send_sem=send_sems.at[p, k - 1], recv_sem=recv_sems.at[p, k - 1],
                device_id=(peer[N_DEV - k],), device_id_type=pl.DeviceIdType.MESH)

        sub_pp = iota((2 * CAP, BLK), 0)

        def sender_pass(p, first):
            if first:
                cp_x.wait()
            for k in range(N_DEV):
                key_row = key_v[p, pl.ds(peer[k], 1), :]
                pp = (sub_pp == key_row).astype(bf16)
                xblk = x_v[pl.ds(pl.multiple_of(peer[k] * BLK, BLK), BLK), :].astype(bf16)
                xx = jnp.dot(pp, xblk, preferred_element_type=f32).astype(bf16)
                lhs_v[k * CAP:(k + 1) * CAP, 0:d_model] = xx[0:CAP]
                lhs_v[k * CAP:(k + 1) * CAP, d_model:2 * d_model] = xx[CAP:2 * CAP]
            acc = None
            for c in range(n_kch):
                if first:
                    cp_w[c].wait()
                wc = w_v[c * KCH:(c + 1) * KCH, :].astype(bf16)
                part = jnp.dot(lhs_v[:, c * KCH:(c + 1) * KCH], wc, preferred_element_type=f32)
                acc = part if acc is None else acc + part
            yb = acc.astype(bf16)
            recv_buf[p, 0:CAP, :] = yb[0:CAP]
            send_buf[p] = yb[CAP:]
            if first:
                pl.semaphore_wait(barrier_sem, N_DEV - 1)
            for k in range(1, N_DEV):
                @pl.when(cnt_send[k] > p * CAP)
                def _():
                    send_copy(p, k).start()

        sender_pass(0, True)
        for p in range(1, N_PASS):
            @pl.when(max_send > p * CAP)
            def _():
                sender_pass(p, False)

        x_own = x_v[pl.ds(pl.multiple_of(me * BLK, BLK), BLK), :]
        cp_rw.wait()
        s_t = lax.dot_general(rwt_v[...], x_own, (((1,), (1,)), ((), ())),
                              preferred_element_type=f32, precision=lax.Precision.HIGHEST)
        s_max = jnp.max(s_t, axis=0, keepdims=True)
        ex = jnp.exp(s_t - s_max)
        p_own = (jnp.sum(jnp.where(iota((n_exp, BLK), 0) == r_own, ex, 0.0), axis=0, keepdims=True)
                 / jnp.sum(ex, axis=0, keepdims=True))
        cp_s.wait()
        shared = jnp.dot(x_own.astype(bf16), sw_v[...].astype(bf16), preferred_element_type=f32)

        rows = iota((N_DEV * CAP, h), 0)
        row_slot = rows // CAP
        row_in_slot = rows % CAP
        sub_q = iota((N_DEV * CAP, BLK), 0)

        def receiver_pass(p):
            rel = rank_own - p * CAP
            keyq = jnp.where((rel >= 0) & (rel < CAP), slot_own * CAP + rel, -1)
            q_t = jnp.where(sub_q == keyq, p_own, 0.0).astype(bf16)
            for k in range(1, N_DEV):
                @pl.when(cnt_recv[k] > p * CAP)
                def _():
                    recv_copy(p, k).wait_recv()
            lim = jnp.full((N_DEV * CAP, h), CAP, i32)
            for k in range(1, N_DEV):
                lim = jnp.where(row_slot == k, n_rows(cnt_recv[k], p), lim)
            rv = jnp.where(row_in_slot < lim, recv_buf[p], jnp.zeros((), bf16))
            return lax.dot_general(q_t, rv, (((0,), (0,)), ((), ())), preferred_element_type=f32)

        out_v[...] = shared + receiver_pass(0)
        for p in range(1, N_PASS):
            @pl.when(max_recv > p * CAP)
            def _():
                out_v[...] = out_v[...] + receiver_pass(p)

        oc = pltpu.make_async_copy(out_v, out_hbm, out_sem)
        oc.start()

        for p in range(N_PASS):
            for k in range(1, N_DEV):
                @pl.when(cnt_send[k] > p * CAP)
                def _():
                    send_copy(p, k).wait_send()
        oc.wait()

    return pl.pallas_call(
        body,
        out_shape=jax.ShapeDtypeStruct((BLK, h), jnp.float32),
        in_specs=[pl.BlockSpec(memory_space=pl.ANY)] * 5,
        out_specs=pl.BlockSpec(memory_space=pl.ANY),
        scratch_shapes=[
            pltpu.VMEM((n_tok, d_model), f32),
            pltpu.VMEM((n_exp, d_model), f32),
            pltpu.VMEM((N_DEV, BLK), i32),
            pltpu.VMEM((k_tot, h), f32),
            pltpu.VMEM((d_model, h), f32),
            pltpu.VMEM((BLK, h), f32),
            pltpu.VMEM((N_PASS, 8, BLK), i32),
            pltpu.VMEM((N_DEV * CAP, k_tot), bf16),
            pltpu.VMEM((N_PASS, (N_DEV - 1) * CAP, h), bf16),
            pltpu.VMEM((N_PASS, N_DEV * CAP, h), bf16),
            pltpu.SemaphoreType.DMA((4 + n_kch,)),
            pltpu.SemaphoreType.DMA,
            pltpu.SemaphoreType.DMA((N_PASS, N_DEV - 1)),
            pltpu.SemaphoreType.DMA((N_PASS, N_DEV - 1)),
        ],
        compiler_params=pltpu.CompilerParams(vmem_limit_bytes=64 * 1024 * 1024, collective_id=0),
    )(x, router_W.T, route_idx.reshape(N_DEV, BLK), expert_W, shared_W)
```

```python
import jax
import jax.numpy as jnp
from jax import lax
from jax.experimental import pallas as pl
from jax.experimental.pallas import tpu as pltpu

N_DEV = 4
BLK = 128
CAP = 64
N_PASS = BLK // CAP
ALIGN = 16
NCH = 2


def pallas_dist_moe_shared_ep_outshard_n512_d256_e2_h512_kernel(
    x: jax.Array,
    router_W: jax.Array,
    route_idx: jax.Array,
    expert_W: jax.Array,
    shared_W: jax.Array,
):
    n_tok, d_model = x.shape
    h = shared_W.shape[1]
    n_exp = router_W.shape[1]
    e_loc = expert_W.shape[0]
    assert n_tok == N_DEV * BLK and e_loc == 2 and h % NCH == 0
    k_tot = e_loc * d_model
    cw = h // NCH
    f32, bf16, i32 = jnp.float32, jnp.bfloat16, jnp.int32

    def iota(shape, dim):
        return lax.broadcasted_iota(i32, shape, dim)

    def body(x_hbm, rwt_hbm, r4_hbm, ew_hbm, sw_hbm, out_hbm,
             x_v, rwt_v, r4_v, w_v, sw_v, out_v, key_v, lhs_v, send_buf, recv_buf,
             r_sem, x_sem, w_sems, late_sems, out_sems, send_sems, recv_sems):
        cp_r = pltpu.make_async_copy(r4_hbm, r4_v, r_sem)
        cp_r.start()

        me = lax.axis_index("i")
        peer = [(me + k) % N_DEV for k in range(N_DEV)]

        barrier_sem = pltpu.get_barrier_semaphore()
        for k in range(1, N_DEV):
            pl.semaphore_signal(barrier_sem, inc=1, device_id=(peer[k],), device_id_type=pl.DeviceIdType.MESH)

        cp_x = pltpu.make_async_copy(x_hbm, x_v, x_sem)
        cp_w = [pltpu.make_async_copy(ew_hbm.at[:, :, pl.ds(c * cw, cw)], w_v.at[c], w_sems.at[c]) for c in range(NCH)]
        cp_rw = pltpu.make_async_copy(rwt_hbm, rwt_v, late_sems.at[0])
        cp_s = pltpu.make_async_copy(sw_hbm, sw_v, late_sems.at[1])
        cp_x.start()

        cp_r.wait()
        for c in cp_w:
            c.start()
        cp_rw.start()
        cp_s.start()

        r4 = r4_v[...]
        r_own = r4_v[pl.ds(me, 1), :]
        sub8 = iota((8, BLK), 0)
        rsel = jnp.broadcast_to(r_own, (8, BLK))
        for d in range(N_DEV):
            rsel = jnp.where(sub8 == d, jnp.broadcast_to(r4[d:d + 1, :], (8, BLK)), rsel)
        g8 = rsel >> 1
        e8 = rsel & 1
        tgt8 = jnp.where(sub8 < N_DEV, me, (me - (sub8 - N_DEV)) & (N_DEV - 1))
        m8 = g8 == tgt8
        m8f = m8.astype(f32)
        upper = (iota((BLK, BLK), 0) < iota((BLK, BLK), 1)).astype(bf16)
        cum8 = jnp.dot(m8f.astype(bf16), upper, preferred_element_type=f32).astype(i32)

        def row_count(row):
            return jnp.sum(jnp.where(sub8 == row, m8f, 0.0)).astype(i32)

        cnt_send = [row_count(peer[k]) for k in range(N_DEV)]
        cnt_recv = [row_count(N_DEV + k) for k in range(N_DEV)]

        def n_rows(cnt, p):
            c = jnp.clip(cnt - p * CAP, 1, CAP)
            return pl.multiple_of(((c + (ALIGN - 1)) // ALIGN) * ALIGN, ALIGN)

        for p in range(N_PASS):
            rel = cum8 - p * CAP
            key_v[p] = jnp.where(m8 & (rel >= 0) & (rel < CAP), rel + CAP * e8, -1)

        rank_own = jnp.sum(jnp.where(sub8 >= N_DEV, cum8 * m8.astype(i32), 0), axis=0, keepdims=True)
        slot_own = (me - (r_own >> 1)) & (N_DEV - 1)

        max_send = jnp.maximum(jnp.maximum(cnt_send[0], cnt_send[1]), jnp.maximum(cnt_send[2], cnt_send[3]))
        max_recv = jnp.maximum(jnp.maximum(cnt_recv[0], cnt_recv[1]), jnp.maximum(cnt_recv[2], cnt_recv[3]))

        def exchange(p, c, k, cnt, dev):
            n = n_rows(cnt, p)
            return pltpu.make_async_remote_copy(
                src_ref=send_buf.at[p, c, pl.ds((k - 1) * CAP, n)],
                dst_ref=recv_buf.at[p, c, pl.ds(k * CAP, n)],
                send_sem=send_sems.at[p, c, k - 1], recv_sem=recv_sems.at[p, c, k - 1],
                device_id=(dev,), device_id_type=pl.DeviceIdType.MESH)

        def send_copy(p, c, k):
            return exchange(p, c, k, cnt_send[k], peer[k])

        def recv_copy(p, c, k):
            return exchange(p, c, k, cnt_recv[k], peer[N_DEV - k])

        sub_pp = iota((2 * CAP, BLK), 0)

        def sender_pass(p, first):
            if first:
                cp_x.wait()
            for d in range(N_DEV):
                pp = (sub_pp == key_v[p, d:d + 1, :]).astype(bf16)
                xblk = x_v[d * BLK:(d + 1) * BLK, :].astype(bf16)
                xx = jnp.dot(pp, xblk, preferred_element_type=f32).astype(bf16)
                region = pl.ds(pl.multiple_of(((d - me) & (N_DEV - 1)) * CAP, CAP), CAP)
                lhs_v[region, 0:d_model] = xx[0:CAP]
                lhs_v[region, d_model:2 * d_model] = xx[CAP:2 * CAP]
            for c in range(NCH):
                if first:
                    cp_w[c].wait()
                wc = w_v[c].reshape(k_tot, cw).astype(bf16)
                yb = jnp.dot(lhs_v[...], wc, preferred_element_type=f32).astype(bf16)
                recv_buf[p, c, 0:CAP, :] = yb[0:CAP]
                send_buf[p, c] = yb[CAP:]
                if first and c == 0:
                    pl.semaphore_wait(barrier_sem, N_DEV - 1)
                for k in range(1, N_DEV):
                    if first:
                        send_copy(p, c, k).start()
                    else:
                        @pl.when(cnt_send[k] > p * CAP)
                        def _():
                            send_copy(p, c, k).start()

        sender_pass(0, True)
        for p in range(1, N_PASS):
            @pl.when(max_send > p * CAP)
            def _():
                sender_pass(p, False)

        x_own = x_v[pl.ds(pl.multiple_of(me * BLK, BLK), BLK), :]
        cp_rw.wait()
        s_t = lax.dot_general(rwt_v[...], x_own, (((1,), (1,)), ((), ())),
                              preferred_element_type=f32, precision=lax.Precision.HIGHEST)
        s_max = jnp.max(s_t, axis=0, keepdims=True)
        ex = jnp.exp(s_t - s_max)
        p_own = (jnp.sum(jnp.where(iota((n_exp, BLK), 0) == r_own, ex, 0.0), axis=0, keepdims=True)
                 / jnp.sum(ex, axis=0, keepdims=True))
        cp_s.wait()
        out_v[...] = jnp.dot(x_own.astype(bf16), sw_v[...].astype(bf16), preferred_element_type=f32)

        rows = iota((N_DEV * CAP, cw), 0)
        row_slot = rows // CAP
        row_in_slot = rows % CAP
        sub_q = iota((N_DEV * CAP, BLK), 0)

        def out_copy(c):
            cols = slice(c * cw, (c + 1) * cw)
            return pltpu.make_async_copy(out_v.at[:, cols], out_hbm.at[:, cols], out_sems.at[c])

        def receiver_pass(p, last):
            rel = rank_own - p * CAP
            keyq = jnp.where((rel >= 0) & (rel < CAP), slot_own * CAP + rel, -1)
            q = jnp.transpose(jnp.where(sub_q == keyq, p_own, 0.0)).astype(bf16)
            lim = jnp.full((N_DEV * CAP, cw), CAP, i32)
            for k in range(1, N_DEV):
                got = n_rows(cnt_recv[k], p)
                if p > 0:
                    got = jnp.where(cnt_recv[k] > p * CAP, got, 0)
                lim = jnp.where(row_slot == k, got, lim)
            valid = row_in_slot < lim
            for c in range(NCH):
                for k in range(1, N_DEV):
                    if p == 0:
                        recv_copy(p, c, k).wait_recv()
                    else:
                        @pl.when(cnt_recv[k] > p * CAP)
                        def _():
                            recv_copy(p, c, k).wait_recv()
                rv = jnp.where(valid, recv_buf[p, c], jnp.zeros((), bf16))
                cols = slice(c * cw, (c + 1) * cw)
                out_v[:, cols] = out_v[:, cols] + jnp.dot(q, rv, preferred_element_type=f32)
                if last:
                    out_copy(c).start()

        for p in range(1, N_PASS):
            @pl.when(max_recv > p * CAP)
            def _():
                receiver_pass(p, False)
        receiver_pass(0, True)

        for c in range(NCH):
            for k in range(1, N_DEV):
                send_copy(0, c, k).wait_send()
        for p in range(1, N_PASS):
            for k in range(1, N_DEV):
                @pl.when(cnt_send[k] > p * CAP)
                def _():
                    for c in range(NCH):
                        send_copy(p, c, k).wait_send()
        for c in range(NCH):
            out_copy(c).wait()

    return pl.pallas_call(
        body,
        out_shape=jax.ShapeDtypeStruct((BLK, h), jnp.float32),
        in_specs=[pl.BlockSpec(memory_space=pl.ANY)] * 5,
        out_specs=pl.BlockSpec(memory_space=pl.ANY),
        scratch_shapes=[
            pltpu.VMEM((n_tok, d_model), f32),
            pltpu.VMEM((n_exp, d_model), f32),
            pltpu.VMEM((N_DEV, BLK), i32),
            pltpu.VMEM((NCH, e_loc, d_model, cw), f32),
            pltpu.VMEM((d_model, h), f32),
            pltpu.VMEM((BLK, h), f32),
            pltpu.VMEM((N_PASS, 8, BLK), i32),
            pltpu.VMEM((N_DEV * CAP, k_tot), bf16),
            pltpu.VMEM((N_PASS, NCH, (N_DEV - 1) * CAP, cw), bf16),
            pltpu.VMEM((N_PASS, NCH, N_DEV * CAP, cw), bf16),
            pltpu.SemaphoreType.DMA,
            pltpu.SemaphoreType.DMA,
            pltpu.SemaphoreType.DMA((NCH,)),
            pltpu.SemaphoreType.DMA((2,)),
            pltpu.SemaphoreType.DMA((NCH,)),
            pltpu.SemaphoreType.DMA((N_PASS, NCH, N_DEV - 1)),
            pltpu.SemaphoreType.DMA((N_PASS, NCH, N_DEV - 1)),
        ],
        compiler_params=pltpu.CompilerParams(vmem_limit_bytes=64 * 1024 * 1024, collective_id=0),
    )(x, router_W.T, route_idx.reshape(N_DEV, BLK), expert_W, shared_W)
```
